```python
import numpy as np

kernel_name = "dist_argmax_global_i_m4096_n1024"

def setup_inputs():
    return {"x": np.random.randn(16384, 1024).astype(np.float32)}

def reference(x: np.ndarray) -> np.ndarray:
    idx = np.argmax(x, axis=0).astype(np.float32)
    val = np.max(x, axis=0)
    return np.stack([val, idx], axis=0)
```

```python
import functools

import jax
import jax.numpy as jnp
from jax import lax
from jax.experimental import pallas as pl
from jax.experimental.pallas import tpu as pltpu

_N_DEV = 4
_SUB = 8
_LANES = 128
_UNROLL = 4
_BIG = 3.0e7
_PUSH_TO = (1, 3)
_PUSH_ROWS = 176
_CHUNKS = (2912, 672, 128, 32)


def _isnan(v):
  return v != v


def _merge(cands):
  best = functools.reduce(jnp.maximum, [v for v, _ in cands])
  rows = [jnp.where(jnp.logical_or(v == best, _isnan(v)), i, _BIG) for v, i in cands]
  return best, functools.reduce(jnp.minimum, rows)


def _pair(ref):
  return ref[0:1, :], ref[1:2, :]


def pallas_dist_argmax_global_i_m4096_n1024_kernel(x: jax.Array):
  rows, cols = x.shape
  n_push = len(_PUSH_TO)
  own = rows - n_push * _PUSH_ROWS
  assert sum(_CHUNKS) == own and cols % _LANES == 0
  starts = [sum(_CHUNKS[:c]) for c in range(len(_CHUNKS))]
  n_chunks = len(_CHUNKS)

  def body(x_hbm, out_ref, xbuf, sbuf, fbuf, rbuf, sems, push_recv_sem, recv_sem):
    load_sems = (sems.at[0], sems.at[1])
    push_send_sems = (sems.at[2], sems.at[3])
    send_sems = (sems.at[0], sems.at[1], sems.at[2])

    def load(c):
      span = pl.ds(starts[c], _CHUNKS[c])
      return pltpu.make_async_copy(
          x_hbm.at[span, :], xbuf.at[span, :], load_sems[c % 2])

    load(0).start()
    load(1).start()

    me = lax.axis_index("i")

    def push(k):
      span = pl.ds(own + k * _PUSH_ROWS, _PUSH_ROWS)
      return pltpu.make_async_remote_copy(
          src_ref=x_hbm.at[span, :], dst_ref=xbuf.at[span, :],
          send_sem=push_send_sems[k], recv_sem=push_recv_sem,
          device_id=(lax.rem(me + _PUSH_TO[k], _N_DEV),),
          device_id_type=pl.DeviceIdType.MESH)

    barrier = pltpu.get_barrier_semaphore()
    for d in range(1, _N_DEV):
      pl.semaphore_signal(
          barrier, inc=1, device_id=(lax.rem(me + d, _N_DEV),),
          device_id_type=pl.DeviceIdType.MESH)
    pl.semaphore_wait(barrier, _N_DEV - 1)
    for k in range(n_push):
      push(k).start()

    def step(g, carry):
      vals, idxs, cur = carry
      xv = xbuf[pl.ds(pl.multiple_of(g * _SUB, _SUB), _SUB), :]
      keep = jnp.logical_or(xv <= vals, _isnan(vals))
      new_idx = jnp.tile(cur, (1, cols // _LANES))
      return (jnp.where(keep, vals, xv), jnp.where(keep, idxs, new_idx),
              cur + float(_SUB))

    sub = lax.broadcasted_iota(jnp.int32, (_SUB, _LANES), 0)

    def init(first_row):
      cur = (sub + first_row).astype(jnp.float32)
      return (jnp.full((_SUB, cols), -jnp.inf, jnp.float32),
              jnp.tile(cur, (1, cols // _LANES)), cur)

    def scan(state, first, n):
      return lax.fori_loop(first // _SUB, (first + n) // _SUB, step, state,
                           unroll=min(_UNROLL, n // _SUB))

    def fold(state, dst):
      vals, idxs, _ = state
      best = jnp.max(vals, axis=0, keepdims=True)
      cand = jnp.logical_or(vals == best, _isnan(vals))
      dst[0:1, :] = best
      dst[1:2, :] = jnp.min(jnp.where(cand, idxs, _BIG), axis=0, keepdims=True)

    state = init(me * rows)
    for c in range(n_chunks):
      load(c).wait()
      if c + 2 < n_chunks:
        load(c + 2).start()
      state = scan(state, starts[c], _CHUNKS[c])
      if c == 0:
        tail = xbuf.at[pl.ds(own, n_push * _PUSH_ROWS), :]
        pltpu.make_async_copy(tail, tail, push_recv_sem).wait()
        for k in range(n_push):
          src = lax.rem(me + (_N_DEV - _PUSH_TO[k]), _N_DEV)
          first = own + k * _PUSH_ROWS
          fold(scan(init(src * rows + first), first, _PUSH_ROWS), fbuf.at[k])
        v, i = _merge([_pair(fbuf.at[k]) for k in range(n_push)])
        fbuf[0, 0:1, :] = v
        fbuf[0, 1:2, :] = i
      if c == n_chunks - 2:
        for k in range(n_push):
          push(k).wait_send()

    fold(state, sbuf)
    v, i = _merge([_pair(sbuf), _pair(fbuf.at[0])])
    sbuf[0:1, :] = v
    sbuf[1:2, :] = i

    def send(d):
      return pltpu.make_async_remote_copy(
          src_ref=sbuf, dst_ref=rbuf.at[d - 1],
          send_sem=send_sems[d - 1], recv_sem=recv_sem,
          device_id=(lax.rem(me + d, _N_DEV),),
          device_id_type=pl.DeviceIdType.MESH)

    for d in (2, 1, 3):
      send(d).start()
    pltpu.make_async_copy(rbuf, rbuf, recv_sem).wait()
    v, i = _merge([_pair(sbuf)] + [_pair(rbuf.at[s]) for s in range(_N_DEV - 1)])
    out_ref[0:1, :] = v
    out_ref[1:2, :] = i
    for d in (2, 1, 3):
      send(d).wait_send()

  return pl.pallas_call(
      body,
      out_shape=jax.ShapeDtypeStruct((2, cols), jnp.float32),
      in_specs=[pl.BlockSpec(memory_space=pl.ANY)],
      out_specs=pl.BlockSpec(memory_space=pltpu.VMEM),
      scratch_shapes=[
          pltpu.VMEM((rows, cols), jnp.float32),
          pltpu.VMEM((2, cols), jnp.float32),
          pltpu.VMEM((n_push, 2, cols), jnp.float32),
          pltpu.VMEM((_N_DEV - 1, 2, cols), jnp.float32),
          pltpu.SemaphoreType.DMA((4,)),
          pltpu.SemaphoreType.DMA,
          pltpu.SemaphoreType.DMA,
      ],
      compiler_params=pltpu.CompilerParams(
          collective_id=0, vmem_limit_bytes=48 * 1024 * 1024),
  )(x)
```
